```python
import numpy as np

kernel_name = "dist_sparse_attn_blocksparse_qseq_b2_sq256_skv256_hq4_dh64"

def setup_inputs():
    x = np.random.randn(2, 1024, 512).astype(np.float32)
    Wq = np.random.randn(512, 1024).astype(np.float32) * 0.02
    K_ext = np.random.randn(2, 256, 16, 64).astype(np.float32)
    V_ext = np.random.randn(2, 256, 16, 64).astype(np.float32)
    Wo = np.random.randn(1024, 512).astype(np.float32) * 0.02
    return {"x": x, "Wq": Wq, "K_ext": K_ext, "V_ext": V_ext, "Wo": Wo}

def reference(x, Wq, K_ext, V_ext, Wo):
    B, Sq, Skv, Hq, Dh = 2, 1024, 256, 16, 64
    Q = (x @ Wq).reshape(B, Sq, Hq, Dh)
    qb = (np.arange(Sq) // 64)[:, None]
    kb = (np.arange(Skv) // 64)[None, :]
    mask = (qb == kb) | (kb == 0) | ((qb + kb) % 3 == 0)
    scores = np.einsum('bihd,bjhd->bhij', Q, K_ext).astype(np.float32) * 0.125
    scores = np.where(mask[None, None, :, :], scores, -1e9)
    scores_max = scores.max(axis=-1, keepdims=True)
    w = np.exp(scores - scores_max)
    row_keep = mask.any(axis=1)
    w_sum = np.where(row_keep[None, None, :, None], w.sum(axis=-1, keepdims=True), 1.0)
    w = w / w_sum
    w = np.where(row_keep[None, None, :, None], w, 0.0)
    ctx = np.einsum('bhij,bjhd->bihd', w, V_ext).reshape(B, Sq, Hq * Dh)
    return ctx @ Wo
```

```python
import contextlib

import jax
import jax.numpy as jnp
from jax import lax
from jax.experimental import pallas as pl
from jax.experimental.pallas import tpu as pltpu

N_DEV = 4
B, SQ, D, SKV, DH = 2, 256, 512, 256, 64
ROWS = B * SQ
BLK = 64
BF16 = jnp.bfloat16
F32 = jnp.float32
MESH = pl.DeviceIdType.MESH
ME, RIGHT, DIAG, LEFT = 0, 1, 2, 3
NT = (((1,), (1,)), ((), ()))


def make_kernel(scopes=False, out_dtype=BF16, head=16, cuts=(64, 192, 512), msplit=4, flags=None):
    scope = jax.named_scope if scopes else (lambda name: contextlib.nullcontext())

    def body(x_hbm, wq_hbm, k_hbm, v_hbm, wo_hbm, out_ref,
             xf, xb, wqf, wof, wqh, wq, wo, kf, vf, ctx, acc,
             lsem, ssem, rsem, ready):
        n_l = [0]

        def local(src, dst):
            cp = pltpu.make_async_copy(src, dst, lsem.at[n_l[0]])
            n_l[0] += 1
            cp.start()
            return cp

        bounds = [0] + list(cuts)
        ld_wq = [local(wq_hbm.at[pl.ds(0, cuts[0])], wqf.at[pl.ds(0, cuts[0])])]

        me = lax.axis_index("i")
        right = (me + 1) & (N_DEV - 1)
        left = (me + 3) & (N_DEV - 1)
        odd = (me & 1) == 1

        bar = pltpu.get_barrier_semaphore()

        @pl.when(me != 2)
        def _():
            for nbr in (left, right):
                pl.semaphore_signal(bar, inc=1, device_id=(nbr,), device_id_type=MESH)

        n_r = [0]
        all_remote = []

        def remote(src, dst, dev):
            i = n_r[0]
            n_r[0] += 1
            cp = pltpu.make_async_remote_copy(src, dst, ssem.at[i], rsem.at[i],
                                              device_id=(dev,), device_id_type=MESH)
            all_remote.append(cp)
            return cp

        def to_right(src, dst):
            return remote(src, dst, right)

        def to_left(src, dst):
            return remote(src, dst, left)

        if head:
            h_r = [to_right(wq_hbm.at[pl.ds(0, head)], wqh.at[0])]
            h_l = [to_left(wq_hbm.at[pl.ds(0, head)], wqh.at[1])]
        else:
            h_r, h_l = [], []
        q_r, q_l = [], []
        for a, b in zip(bounds[:-1], bounds[1:]):
            a = max(a, head)
            rows = pl.ds(a, b - a)
            q_r.append(to_right(wq.at[ME, 0, rows], wq.at[LEFT, 0, rows]))
            q_l.append(to_left(wq.at[ME, 1, rows], wq.at[RIGHT, 1, rows]))
        rest = pl.ds(head, D - head)
        q2_r = to_right(wq.at[ME, 1, rest], wq.at[LEFT, 1, rest])
        q2_l = to_left(wq.at[ME, 0, rest], wq.at[RIGHT, 0, rest])
        o1_r = to_right(wo.at[ME, 0], wo.at[LEFT, 0])
        o1_l = to_left(wo.at[ME, 1], wo.at[RIGHT, 1])
        qf_r = to_right(wq.at[LEFT, 0], wq.at[DIAG, 0])
        qf_l = to_left(wq.at[RIGHT, 1], wq.at[DIAG, 1])
        o2_r = to_right(wo.at[ME, 1], wo.at[LEFT, 1])
        o2_l = to_left(wo.at[ME, 0], wo.at[RIGHT, 0])
        tile_groups = ((0, 2), (2, 2), (4, 2), (6, 1), (7, 1))
        of_r = [to_right(wo.at[LEFT, 0, pl.ds(t, n)], wo.at[DIAG, 0, pl.ds(t, n)]) for t, n in tile_groups]
        of_l = [to_left(wo.at[RIGHT, 1, pl.ds(t, n)], wo.at[DIAG, 1, pl.ds(t, n)]) for t, n in tile_groups]

        def start(cps):
            for cp in cps:
                cp.start()

        def early(cps_r, cps_l):
            @pl.when(me >= 2)
            def _():
                start(cps_r)

            @pl.when((me == 1) | (me == 2))
            def _():
                start(cps_l)

        with scope("barrier"):
            @pl.when(odd)
            def _():
                pl.semaphore_wait(bar, 1)

            @pl.when(me == 2)
            def _():
                pl.semaphore_wait(bar, 2)
                for nbr in (left, right):
                    pl.semaphore_signal(ready, inc=1, device_id=(nbr,), device_id_type=MESH)
        early(h_r, h_l)

        for a, b in zip(bounds[1:-1], bounds[2:]):
            ld_wq.append(local(wq_hbm.at[pl.ds(a, b - a)], wqf.at[pl.ds(a, b - a)]))
        ld_wo = local(wo_hbm, wof)
        ld_x = local(x_hbm, xf)
        ld_kv = {}
        for slot, hp in ((ME, 0), (ME, 1), (LEFT, 0), (RIGHT, 1), (LEFT, 1), (RIGHT, 0), (DIAG, 0), (DIAG, 1)):
            row0 = pl.multiple_of(((me + slot) & (N_DEV - 1)) * 256 + hp * 128, 128)
            ld_kv[slot, hp] = (local(k_hbm.at[:, pl.ds(row0, 128), :], kf.at[slot, hp]),
                               local(v_hbm.at[:, pl.ds(row0, 128), :], vf.at[slot, hp]))

        for i, (a, b) in enumerate(zip(bounds[:-1], bounds[1:])):
            with scope(f"wq{i}"):
                ld_wq[i].wait()
                w = wqf[pl.ds(a, b - a), :].astype(BF16)
                wq[ME, 0, pl.ds(a, b - a), :] = w[:, :128]
                wq[ME, 1, pl.ds(a, b - a), :] = w[:, 128:]
            early([q_r[i]], [q_l[i]])
        early([q2_r], [q2_l])

        with scope("ready"):
            @pl.when(me == 0)
            def _():
                pl.semaphore_wait(bar, 2)

            @pl.when(odd)
            def _():
                pl.semaphore_wait(ready, 1)

        @pl.when(me <= 1)
        def _():
            start(h_r + q_r + [q2_r])

        @pl.when((me == 0) | (me == 3))
        def _():
            start(h_l + q_l + [q2_l])

        with scope("wo_cast"):
            ld_wo.wait()
            for kt in range(2):
                for h in range(2):
                    w = wof[pl.ds(kt * 128 + h * DH, DH), :].astype(BF16)
                    for nb in range(4):
                        wo[ME, h, nb * 2 + kt] = w[:, nb * 128:(nb + 1) * 128]
        start([o1_r, o1_l])

        first_head = lax.broadcasted_iota(jnp.int32, (8, 128), 1) < DH
        first_head16 = lax.broadcasted_iota(jnp.int32, (16, 128), 1) < DH
        kb = lax.broadcasted_iota(jnp.int32, (8, SKV), 1) // BLK
        masks = []
        for j in range(SQ // BLK):
            qb = me * (SQ // BLK) + j
            masks.append((qb == kb) | (kb == 0) | ((qb + kb) % 3 == 0))
        zeros = jnp.zeros((DH, SKV), BF16)
        ones = jnp.ones((DH, SKV), BF16)

        def qproj(key):
            return (jnp.dot(xb[...], wq[key], preferred_element_type=F32) * 0.125).astype(BF16)

        def qk(key, b, q):
            kt = kf[key[0], key[1], b].astype(BF16)
            kz = jnp.concatenate([jnp.concatenate([kt[:DH], zeros], 0),
                                  jnp.concatenate([zeros, kt[DH:]], 0)], 1)
            return jnp.dot(q[b * SQ:(b + 1) * SQ], kz, preferred_element_type=F32)

        def softmax_num(s):
            out = []
            for h in range(2):
                ps = []
                for j in range(SQ // BLK):
                    sj = s[j * BLK:(j + 1) * BLK, h * SKV:(h + 1) * SKV].reshape(BLK // 8, 8, SKV)
                    sj = jnp.where(masks[j][None], sj, -1e9)
                    m = jnp.max(sj, axis=2, keepdims=True)
                    ps.append(jnp.exp(sj - m).reshape(BLK, SKV).astype(BF16))
                out.append(jnp.concatenate(ps, 0))
            return out

        def pv(key, b, p):
            vt = vf[key[0], key[1], b].astype(BF16)
            r0 = lax.dot_general(p[0], jnp.concatenate([vt[:DH], ones], 0), NT,
                                 preferred_element_type=F32).reshape(SQ // 8, 8, 128)
            r1 = lax.dot_general(p[1], jnp.concatenate([ones, vt[DH:]], 0), NT,
                                 preferred_element_type=F32).reshape(SQ // 8, 8, 128)
            c = jnp.where(first_head[None], r0, r1).reshape(SQ, 128)
            l = pltpu.roll(jnp.where(first_head[None], r1, r0).reshape(SQ, 128), DH, 1)
            ctx[key[0], key[1], pl.ds(b * SQ, SQ), :] = (c / l).astype(BF16)

        def attend(*keys):
            for key in keys:
                for cp in ld_kv[key]:
                    cp.wait()
            q = qproj(keys[0])
            s0 = qk(keys[0], 0, q)
            for u, key in enumerate(keys):
                s1 = qk(key, 1, q)
                p0 = softmax_num(s0)
                if u + 1 < len(keys):
                    q = qproj(keys[u + 1])
                pv(key, 0, p0)
                p1 = softmax_num(s1)
                if u + 1 < len(keys):
                    s0 = qk(keys[u + 1], 0, q)
                pv(key, 1, p1)

        def wo_tile(s0, s1, t):
            return jnp.concatenate([wo[s0, 0, t], wo[s1, 1, t]], axis=0)

        def ctx_tile(s0, s1, kt):
            if s0 == s1:
                return ctx[s0, kt]
            a = ctx[s0, kt].reshape(ROWS // 16, 16, 128)
            b = ctx[s1, kt].reshape(ROWS // 16, 16, 128)
            return jnp.where(first_head16[None], a, b).reshape(ROWS, 128)

        def proj(pairs):
            lhs = jnp.concatenate([ctx_tile(s0, s1, kt) for s0, s1 in pairs for kt in range(2)], axis=1)
            rhs = jnp.concatenate(
                [jnp.concatenate([wo_tile(s0, s1, nb * 2 + kt) for nb in range(4)], axis=1)
                 for s0, s1 in pairs for kt in range(2)], axis=0)
            return jnp.dot(lhs, rhs, preferred_element_type=F32)

        with scope("x"):
            ld_x.wait()
            xb[...] = xf[...].astype(BF16)
        with scope("att_me"):
            attend((ME, 0), (ME, 1))
        with scope("wait1"):
            for cp in h_r + h_l + q_r + q_l:
                cp.wait_recv()
            if head:
                for i, slot in enumerate((LEFT, RIGHT)):
                    w = wqh[i].astype(BF16)
                    wq[slot, 0, pl.ds(0, head), :] = w[:, :128]
                    wq[slot, 1, pl.ds(0, head), :] = w[:, 128:]
        start([qf_r, qf_l, o2_r, o2_l])
        with scope("att1"):
            attend((LEFT, 0), (RIGHT, 1))
        with scope("wait2"):
            q2_r.wait_recv()
            q2_l.wait_recv()
        with scope("att2"):
            attend((LEFT, 1), (RIGHT, 0))
        with scope("wait3"):
            o1_r.wait_recv()
            o1_l.wait_recv()
        for a, b in zip(of_r, of_l):
            start([a, b])
        with scope("proj1"):
            acc[...] = proj(((ME, ME), (LEFT, RIGHT)))
        with scope("wait4"):
            qf_r.wait_recv()
            qf_l.wait_recv()
        with scope("att3"):
            attend((DIAG, 0), (DIAG, 1))
        with scope("wait5"):
            o2_r.wait_recv()
            o2_l.wait_recv()
        with scope("proj2"):
            acc[...] += proj(((RIGHT, LEFT),))
        late = [of_r[-1], of_l[-1], of_r[-2], of_l[-2]]
        for g, (t, n) in enumerate(tile_groups):
            if g == len(tile_groups) - 2:
                with scope("wait_send"):
                    for cp in all_remote:
                        if not any(cp is c for c in late):
                            cp.wait_send()
            if g == len(tile_groups) - 1:
                for cp in late:
                    cp.wait_send()
            with scope(f"wait6_{g}"):
                of_r[g].wait_recv()
                of_l[g].wait_recv()
            with scope(f"proj3_{g}"):
                nb = t // 2
                cols = pl.ds(nb * 128, 128)
                rhs = jnp.concatenate([wo_tile(DIAG, DIAG, t + i) for i in range(n)], axis=0)
                parts = msplit // n
                for mi in range(parts):
                    rows = pl.ds(mi * (ROWS // parts), ROWS // parts)
                    lhs = jnp.concatenate([ctx[DIAG, (t + i) % 2, rows, :] for i in range(n)], axis=1)
                    r = acc[rows, cols] + jnp.dot(lhs, rhs, preferred_element_type=F32)
                    if (t + n) % 2 == 0:
                        out_ref[rows, cols] = r.astype(out_dtype)
                    else:
                        acc[rows, cols] = r

    def kernel(x, Wq, K_ext, V_ext, Wo):
        x2 = x.reshape(ROWS, D)
        kt = K_ext.transpose(0, 2, 3, 1).reshape(B, 16 * DH, SKV)
        vt = V_ext.transpose(0, 2, 3, 1).reshape(B, 16 * DH, SKV)
        hbm = pl.BlockSpec(memory_space=pltpu.HBM)
        out = pl.pallas_call(
            body,
            out_shape=jax.ShapeDtypeStruct((ROWS, D), out_dtype),
            in_specs=[hbm] * 5,
            out_specs=pl.BlockSpec(memory_space=pltpu.VMEM),
            scratch_shapes=[
                pltpu.VMEM((ROWS, D), F32),
                pltpu.VMEM((ROWS, D), BF16),
                pltpu.VMEM((D, 256), F32),
                pltpu.VMEM((256, D), F32),
                pltpu.VMEM((2, max(head, 8), 256), F32),
                pltpu.VMEM((4, 2, D, 128), BF16),
                pltpu.VMEM((4, 2, 8, DH, 128), BF16),
                pltpu.VMEM((4, 2, B, 128, SKV), F32),
                pltpu.VMEM((4, 2, B, 128, SKV), F32),
                pltpu.VMEM((4, 2, ROWS, 128), BF16),
                pltpu.VMEM((ROWS, D), F32),
                pltpu.SemaphoreType.DMA((24,)),
                pltpu.SemaphoreType.DMA((32,)),
                pltpu.SemaphoreType.DMA((32,)),
                pltpu.SemaphoreType.REGULAR,
            ],
            compiler_params=pltpu.CompilerParams(
                collective_id=0, disable_bounds_checks=True, disable_semaphore_checks=True, flags=flags),
        )(x2, Wq, kt, vt, Wo)
        return out.reshape(B, SQ, D)

    return kernel


def pallas_dist_sparse_attn_blocksparse_qseq_b2_sq256_skv256_hq4_dh64_kernel(x, Wq, K_ext, V_ext, Wo):
    return make_kernel()(x, Wq, K_ext, V_ext, Wo)
```

```python
import jax
import jax.numpy as jnp
from jax import lax
from jax.experimental import pallas as pl
from jax.experimental.pallas import tpu as pltpu

N_DEV = 4
B, SQ, D = 2, 256, 512
SKV, DH = 256, 64
HEADS = 4
PAIR = 2 * DH
ROWS = B * SQ
BLK = 64
BF16, F32 = jnp.bfloat16, jnp.float32

ME, RIGHT, DIAG, LEFT = range(N_DEV)

HEAD = 16
WQ_CUTS = (0, 32, 96, 256, D)
WO_PIECES = ((0, 2), (2, 2), (4, 2), (6, 1), (7, 1))
KV_ORDER = ((ME, 0), (ME, 1), (LEFT, 0), (RIGHT, 1),
            (LEFT, 1), (RIGHT, 0), (DIAG, 0), (DIAG, 1))

N_LOCAL = (len(WQ_CUTS) - 1) + 2 + 2 * len(KV_ORDER)
N_REMOTE = 2 * (1 + (len(WQ_CUTS) - 1) + 4 + len(WO_PIECES))


def _body(x_hbm, wq_hbm, k_hbm, v_hbm, wo_hbm, out_ref,
          x_f32, x_bf, wq_f32, wo_f32, wq_head, wq, wo, kt, vt, ctx, acc,
          local_sems, send_sems, recv_sems, ready_sem):
    local_copies, remote_copies = [], []

    def load(src, dst):
        copy = pltpu.make_async_copy(src, dst, local_sems.at[len(local_copies)])
        local_copies.append(copy)
        copy.start()
        return copy

    wq_rows = [pl.ds(a, b - a) for a, b in zip(WQ_CUTS[:-1], WQ_CUTS[1:])]
    wq_loads = [load(wq_hbm.at[wq_rows[0]], wq_f32.at[wq_rows[0]])]

    me = lax.axis_index("i")
    right = (me + 1) & (N_DEV - 1)
    left = (me + 3) & (N_DEV - 1)

    def signal_neighbours(sem):
        for neighbour in (left, right):
            pl.semaphore_signal(sem, inc=1, device_id=(neighbour,),
                                device_id_type=pl.DeviceIdType.MESH)

    def remote(src, dst, device):
        i = len(remote_copies)
        copy = pltpu.make_async_remote_copy(
            src, dst, send_sems.at[i], recv_sems.at[i],
            device_id=(device,), device_id_type=pl.DeviceIdType.MESH)
        remote_copies.append(copy)
        return copy

    def both_ways(src_cw, dst_cw, src_ccw, dst_ccw):
        return remote(src_cw, dst_cw, right), remote(src_ccw, dst_ccw, left)

    def start(*pairs):
        for pair in pairs:
            for copy in pair:
                copy.start()

    def arrived(*pairs):
        for pair in pairs:
            for copy in pair:
                copy.wait_recv()

    head = both_ways(wq_hbm.at[pl.ds(0, HEAD)], wq_head.at[0],
                     wq_hbm.at[pl.ds(0, HEAD)], wq_head.at[1])
    wq_first = []
    for a, b in zip(WQ_CUTS[:-1], WQ_CUTS[1:]):
        rows = pl.ds(max(a, HEAD), b - max(a, HEAD))
        wq_first.append(both_ways(wq.at[ME, 0, rows], wq.at[LEFT, 0, rows],
                                  wq.at[ME, 1, rows], wq.at[RIGHT, 1, rows]))
    rows = pl.ds(HEAD, D - HEAD)
    wq_second = both_ways(wq.at[ME, 1, rows], wq.at[LEFT, 1, rows],
                          wq.at[ME, 0, rows], wq.at[RIGHT, 0, rows])
    wo_first = both_ways(wo.at[ME, 0], wo.at[LEFT, 0], wo.at[ME, 1], wo.at[RIGHT, 1])
    wq_forward = both_ways(wq.at[LEFT, 0], wq.at[DIAG, 0], wq.at[RIGHT, 1], wq.at[DIAG, 1])
    wo_second = both_ways(wo.at[ME, 1], wo.at[LEFT, 1], wo.at[ME, 0], wo.at[RIGHT, 0])
    wo_forward = [both_ways(wo.at[LEFT, 0, pl.ds(t, n)], wo.at[DIAG, 0, pl.ds(t, n)],
                            wo.at[RIGHT, 1, pl.ds(t, n)], wo.at[DIAG, 1, pl.ds(t, n)])
                  for t, n in WO_PIECES]

    barrier = pltpu.get_barrier_semaphore()
    odd = (me & 1) == 1

    @pl.when(me != 2)
    def _():
        signal_neighbours(barrier)

    @pl.when(odd)
    def _():
        pl.semaphore_wait(barrier, 1)

    @pl.when(me == 2)
    def _():
        pl.semaphore_wait(barrier, 2)
        signal_neighbours(ready_sem)

    def start_on_open_links(pair):
        @pl.when(me >= 2)
        def _():
            pair[0].start()

        @pl.when((me == 1) | (me == 2))
        def _():
            pair[1].start()

    start_on_open_links(head)

    wq_loads += [load(wq_hbm.at[rows], wq_f32.at[rows]) for rows in wq_rows[1:]]
    wo_load = load(wo_hbm, wo_f32)
    x_load = load(x_hbm, x_f32)
    kv_loads = {}
    for slot, pair in KV_ORDER:
        heads = pl.ds(((me + slot) & (N_DEV - 1)) * HEADS + 2 * pair, 2)
        kv_loads[slot, pair] = (load(k_hbm.at[:, heads], kt.at[slot, pair]),
                                load(v_hbm.at[:, heads], vt.at[slot, pair]))

    for rows, wq_load, piece in zip(wq_rows, wq_loads, wq_first):
        wq_load.wait()
        w = wq_f32[rows, :].astype(BF16)
        wq[ME, 0, rows, :] = w[:, :PAIR]
        wq[ME, 1, rows, :] = w[:, PAIR:]
        start_on_open_links(piece)
    start_on_open_links(wq_second)

    @pl.when(me == 0)
    def _():
        pl.semaphore_wait(barrier, 2)

    @pl.when(odd)
    def _():
        pl.semaphore_wait(ready_sem, 1)

    @pl.when(me <= 1)
    def _():
        for pair in (head, *wq_first, wq_second):
            pair[0].start()

    @pl.when((me == 0) | (me == 3))
    def _():
        for pair in (head, *wq_first, wq_second):
            pair[1].start()

    wo_load.wait()
    for pair in range(2):
        for h in range(2):
            w = wo_f32[pl.ds(pair * PAIR + h * DH, DH), :].astype(BF16)
            for cb in range(D // 128):
                wo[ME, h, 2 * cb + pair] = w[:, cb * 128:(cb + 1) * 128]
    start(wo_first)

    kb = lax.broadcasted_iota(jnp.int32, (8, SKV), 1) // BLK
    masks = []
    for j in range(SQ // BLK):
        qb = me * (SQ // BLK) + j
        masks.append((qb == kb) | (kb == 0) | ((qb + kb) % 3 == 0))
    zeros = jnp.zeros((DH, SKV), BF16)
    ones = jnp.ones((DH, SKV), BF16)

    def by_head(a, b):
        sub = 8 * 4 // a.dtype.itemsize
        first = lax.broadcasted_iota(jnp.int32, (1, sub, PAIR), 2) < DH
        return jnp.where(first, a.reshape(-1, sub, PAIR),
                         b.reshape(-1, sub, PAIR)).reshape(a.shape)

    def queries(key):
        q = jnp.dot(x_bf[...], wq[key], preferred_element_type=F32)
        return (q * 0.125).astype(BF16)

    def scores(key, b, q):
        k0, k1 = (kt[key[0], key[1], b, h].astype(BF16) for h in range(2))
        k = jnp.concatenate([jnp.concatenate([k0, zeros], axis=0),
                             jnp.concatenate([zeros, k1], axis=0)], axis=1)
        return jnp.dot(q[b * SQ:(b + 1) * SQ], k, preferred_element_type=F32)

    def exp_scores(s):
        out = []
        for h in range(2):
            blocks = []
            for j in range(SQ // BLK):
                sj = s[j * BLK:(j + 1) * BLK, h * SKV:(h + 1) * SKV]
                sj = jnp.where(masks[j][None], sj.reshape(BLK // 8, 8, SKV), -1e9)
                p = jnp.exp(sj - jnp.max(sj, axis=2, keepdims=True))
                blocks.append(p.reshape(BLK, SKV).astype(BF16))
            out.append(jnp.concatenate(blocks, axis=0))
        return out

    def context(key, b, p):
        v0, v1 = (vt[key[0], key[1], b, h].astype(BF16) for h in range(2))
        nt = (((1,), (1,)), ((), ()))
        r0 = lax.dot_general(p[0], jnp.concatenate([v0, ones], axis=0), nt,
                             preferred_element_type=F32)
        r1 = lax.dot_general(p[1], jnp.concatenate([ones, v1], axis=0), nt,
                             preferred_element_type=F32)
        total = pltpu.roll(by_head(r1, r0), DH, 1)
        ctx[key[0], key[1], pl.ds(b * SQ, SQ), :] = (by_head(r0, r1) / total).astype(BF16)

    def attend(*keys):
        for key in keys:
            for copy in kv_loads[key]:
                copy.wait()
        q = queries(keys[0])
        s0 = scores(keys[0], 0, q)
        for key, following in zip(keys, (*keys[1:], None)):
            s1 = scores(key, 1, q)
            p0 = exp_scores(s0)
            if following is not None:
                q = queries(following)
            context(key, 0, p0)
            p1 = exp_scores(s1)
            if following is not None:
                s0 = scores(following, 0, q)
            context(key, 1, p1)

    def wo_tile(slot0, slot1, tile):
        return jnp.concatenate([wo[slot0, 0, tile], wo[slot1, 1, tile]], axis=0)

    def project(*slots):
        lhs = [ctx[s0, pair] if s0 == s1 else by_head(ctx[s0, pair], ctx[s1, pair])
               for s0, s1 in slots for pair in range(2)]
        rhs = [jnp.concatenate([wo_tile(s0, s1, 2 * cb + pair) for cb in range(D // 128)],
                               axis=1)
               for s0, s1 in slots for pair in range(2)]
        return jnp.dot(jnp.concatenate(lhs, axis=1), jnp.concatenate(rhs, axis=0),
                       preferred_element_type=F32)

    x_load.wait()
    x_bf[...] = x_f32[...].reshape(ROWS, D).astype(BF16)
    attend((ME, 0), (ME, 1))

    arrived(head, *wq_first)
    for i, slot in enumerate((LEFT, RIGHT)):
        w = wq_head[i].astype(BF16)
        wq[slot, 0, pl.ds(0, HEAD), :] = w[:, :PAIR]
        wq[slot, 1, pl.ds(0, HEAD), :] = w[:, PAIR:]
    start(wq_forward, wo_second)
    attend((LEFT, 0), (RIGHT, 1))

    arrived(wq_second)
    attend((LEFT, 1), (RIGHT, 0))

    arrived(wo_first)
    start(*wo_forward)
    acc[...] = project((ME, ME), (LEFT, RIGHT))

    arrived(wq_forward)
    attend((DIAG, 0), (DIAG, 1))

    arrived(wo_second)
    acc[...] += project((RIGHT, LEFT))

    for piece, (tile, count) in zip(wo_forward, WO_PIECES):
        if piece is wo_forward[-1]:
            for copy in remote_copies:
                copy.wait_send()
        arrived(piece)
        cols = pl.ds(tile // 2 * 128, 128)
        rhs = jnp.concatenate([wo_tile(DIAG, DIAG, tile + i) for i in range(count)], axis=0)
        parts = 4 // count
        for part in range(parts):
            rows = pl.ds(part * (ROWS // parts), ROWS // parts)
            lhs = jnp.concatenate(
                [ctx[DIAG, (tile + i) % 2, rows, :] for i in range(count)], axis=1)
            total = acc[rows, cols] + jnp.dot(lhs, rhs, preferred_element_type=F32)
            if (tile + count) % 2 == 0:
                out_ref[rows, cols] = total.astype(out_ref.dtype)
            else:
                acc[rows, cols] = total


def pallas_dist_sparse_attn_blocksparse_qseq_b2_sq256_skv256_hq4_dh64_kernel(
    x: jax.Array,
    Wq: jax.Array,
    K_ext: jax.Array,
    V_ext: jax.Array,
    Wo: jax.Array,
):
    k_t = K_ext.transpose(0, 2, 3, 1)
    v_t = V_ext.transpose(0, 2, 3, 1)
    out = pl.pallas_call(
        _body,
        out_shape=jax.ShapeDtypeStruct((ROWS, D), BF16),
        in_specs=[pl.BlockSpec(memory_space=pltpu.HBM)] * 5,
        out_specs=pl.BlockSpec(memory_space=pltpu.VMEM),
        scratch_shapes=[
            pltpu.VMEM((B, SQ, D), F32),
            pltpu.VMEM((ROWS, D), BF16),
            pltpu.VMEM((D, HEADS * DH), F32),
            pltpu.VMEM((HEADS * DH, D), F32),
            pltpu.VMEM((2, HEAD, HEADS * DH), F32),
            pltpu.VMEM((N_DEV, 2, D, PAIR), BF16),
            pltpu.VMEM((N_DEV, 2, 8, DH, 128), BF16),
            pltpu.VMEM((N_DEV, 2, B, 2, DH, SKV), F32),
            pltpu.VMEM((N_DEV, 2, B, 2, DH, SKV), F32),
            pltpu.VMEM((N_DEV, 2, ROWS, PAIR), BF16),
            pltpu.VMEM((ROWS, D), F32),
            pltpu.SemaphoreType.DMA((N_LOCAL,)),
            pltpu.SemaphoreType.DMA((N_REMOTE,)),
            pltpu.SemaphoreType.DMA((N_REMOTE,)),
            pltpu.SemaphoreType.REGULAR,
        ],
        compiler_params=pltpu.CompilerParams(
            collective_id=0,
            disable_semaphore_checks=True,
        ),
    )(x, Wq, k_t, v_t, Wo)
    return out.reshape(B, SQ, D)
```
